```python
import numpy as np

kernel_name = "dist_layernorm_xy_m512_n256"

def setup_inputs():
    x = np.random.randn(1024, 512).astype(np.float32)
    gamma = np.random.randn(512).astype(np.float32)
    beta = np.random.randn(512).astype(np.float32)
    return {"x": x, "gamma": gamma, "beta": beta}

def reference(x: np.ndarray, gamma: np.ndarray, beta: np.ndarray) -> np.ndarray:
    eps = 1e-5
    mean = np.mean(x, axis=1, keepdims=True)
    var = np.var(x, axis=1, keepdims=True)
    return gamma * (x - mean) / np.sqrt(var + eps) + beta
```

```python
import jax
import jax.numpy as jnp
from jax import lax
from jax.experimental import pallas as pl
from jax.experimental.pallas import tpu as pltpu

M, N = 512, 256
EPS = 1e-5
CHUNKS = (128, 128, 128, 128)
assert sum(CHUNKS) == M and all(r <= 128 and r % 8 == 0 for r in CHUNKS)
STARTS = tuple(sum(CHUNKS[:i]) for i in range(len(CHUNKS)))
C = len(CHUNKS)
MESH = pl.DeviceIdType.MESH


def pallas_dist_layernorm_xy_m512_n256_kernel(x, gamma, beta):
    def body(x_hbm, g_hbm, b_hbm, o_ref, xv, gv, bv, st, rx, in_sems, p_sems, send_sems, recv_sems):
        in_cps = [
            pltpu.make_async_copy(x_hbm.at[pl.ds(STARTS[c], CHUNKS[c])], xv.at[pl.ds(STARTS[c], CHUNKS[c])], in_sems.at[c])
            for c in range(C)
        ]
        for cp in in_cps:
            cp.start()
        nbr = (lax.axis_index("x"), 1 - lax.axis_index("y"))
        bar = pltpu.get_barrier_semaphore()
        pl.semaphore_signal(bar, inc=1, device_id=nbr, device_id_type=MESH)
        g_cp = pltpu.make_async_copy(g_hbm, gv, p_sems.at[0])
        b_cp = pltpu.make_async_copy(b_hbm, bv, p_sems.at[1])
        g_cp.start()
        b_cp.start()

        diff = (lax.broadcasted_iota(jnp.int32, (8, 128), 1)
                - lax.broadcasted_iota(jnp.int32, (8, 128), 0))

        rdmas = []
        for c in range(C):
            in_cps[c].wait()
            accm = jnp.zeros((8, 128), jnp.float32)
            accq = jnp.zeros((8, 128), jnp.float32)
            for g in range(CHUNKS[c] // 8):
                r0 = STARTS[c] + 8 * g
                xa = xv[r0:r0 + 8, 0:128]
                xb = xv[r0:r0 + 8, 128:256]
                mean = jnp.sum(xa + xb, axis=1, keepdims=True) * (1.0 / N)
                da = xa - mean
                db = xb - mean
                m2 = jnp.sum(da * da + db * db, axis=1, keepdims=True)
                msk = diff == 8 * g
                accm = jnp.where(msk, mean, accm)
                accq = jnp.where(msk, m2, accq)
            st[c, 0:1, :] = jnp.sum(accm, axis=0, keepdims=True)
            st[c, 1:2, :] = jnp.sum(accq, axis=0, keepdims=True)
            if c == 0:
                pl.semaphore_wait(bar, 1)
            rd = pltpu.make_async_remote_copy(
                src_ref=st.at[c], dst_ref=rx.at[c], send_sem=send_sems.at[c], recv_sem=recv_sems.at[c],
                device_id=nbr, device_id_type=MESH)
            rd.start()
            rdmas.append(rd)

        g_cp.wait()
        b_cp.wait()
        ga = gv[:, 0:128]
        gb = gv[:, 128:256]
        ba = bv[:, 0:128]
        bb = bv[:, 128:256]
        for c in range(C):
            rdmas[c].wait_recv()
            m_a = st[c, 0:1, :]
            q_a = st[c, 1:2, :]
            m_b = rx[c, 0:1, :]
            q_b = rx[c, 1:2, :]
            dl = m_a - m_b
            mean = 0.5 * (m_a + m_b)
            var = (q_a + q_b + dl * dl * (N / 2.0)) * (1.0 / (2 * N))
            rstd = lax.rsqrt(var + EPS)
            mean8 = jnp.broadcast_to(mean, (8, 128))
            rstd8 = jnp.broadcast_to(rstd, (8, 128))
            for g in range(CHUNKS[c] // 8):
                r0 = STARTS[c] + 8 * g
                msk = diff == 8 * g
                mu = jnp.sum(jnp.where(msk, mean8, 0.0), axis=1, keepdims=True)
                rs = jnp.sum(jnp.where(msk, rstd8, 0.0), axis=1, keepdims=True)
                o_ref[r0:r0 + 8, 0:128] = (xv[r0:r0 + 8, 0:128] - mu) * rs * ga + ba
                o_ref[r0:r0 + 8, 128:256] = (xv[r0:r0 + 8, 128:256] - mu) * rs * gb + bb
        for rd in rdmas:
            rd.wait_send()

    return pl.pallas_call(
        body,
        out_shape=pltpu.VMEM((M, N), jnp.float32),
        in_specs=[pl.BlockSpec(memory_space=pltpu.HBM)] * 3,
        out_specs=pl.BlockSpec(memory_space=pltpu.VMEM),
        scratch_shapes=[
            pltpu.VMEM((M, N), jnp.float32),
            pltpu.VMEM((1, N), jnp.float32),
            pltpu.VMEM((1, N), jnp.float32),
            pltpu.VMEM((C, 2, 128), jnp.float32),
            pltpu.VMEM((C, 2, 128), jnp.float32),
            pltpu.SemaphoreType.DMA((C,)),
            pltpu.SemaphoreType.DMA((2,)),
            pltpu.SemaphoreType.DMA((C,)),
            pltpu.SemaphoreType.DMA((C,)),
        ],
        compiler_params=pltpu.CompilerParams(collective_id=0),
    )(x, gamma.reshape(1, N), beta.reshape(1, N))
```

```python
import jax
import jax.numpy as jnp
from jax import lax
from jax.experimental import pallas as pl
from jax.experimental.pallas import tpu as pltpu

M, N = 512, 256
EPS = 1e-5
CHUNKS = (136, 128, 128, 120)
STARTS = tuple(sum(CHUNKS[:i]) for i in range(len(CHUNKS)))
C = len(CHUNKS)
TILES = tuple(-(-r // 128) for r in CHUNKS)
TMAX = max(TILES)
PIV = 8
MESH = pl.DeviceIdType.MESH


def pallas_dist_layernorm_xy_m512_n256_kernel(x, gamma, beta):
    def body(x_hbm, g_hbm, b_hbm, o_ref, xv, gv, bv, st, rx, in_sems, p_sems, send_sems, recv_sems):
        bounds = [(0, PIV)] + [(max(STARTS[c], PIV), STARTS[c] + CHUNKS[c]) for c in range(C)]
        in_cps = [
            pltpu.make_async_copy(x_hbm.at[pl.ds(a, b - a)], xv.at[pl.ds(a, b - a)], in_sems.at[i])
            for i, (a, b) in enumerate(bounds)
        ]
        for cp in in_cps:
            cp.start()
        nbr = (lax.axis_index("x"), 1 - lax.axis_index("y"))
        bar = pltpu.get_barrier_semaphore()
        pl.semaphore_signal(bar, inc=1, device_id=nbr, device_id_type=MESH)
        g_cp = pltpu.make_async_copy(g_hbm, gv, p_sems.at[0])
        b_cp = pltpu.make_async_copy(b_hbm, bv, p_sems.at[1])
        g_cp.start()
        b_cp.start()

        diff = (lax.broadcasted_iota(jnp.int32, (8, 128), 1)
                - lax.broadcasted_iota(jnp.int32, (8, 128), 0))

        in_cps[0].wait()
        pivot = jnp.sum(xv[0:PIV, 0:128] + xv[0:PIV, 128:256], axis=1, keepdims=True) * (1.0 / N)
        pivot = jnp.broadcast_to(pivot, (8, 128))
        half_pivot_row = jnp.sum(jnp.where((diff & 7) == 0, pivot * 0.5, 0.0), axis=0, keepdims=True)

        rdmas = []
        for c in range(C):
            in_cps[c + 1].wait()
            for t in range(TILES[c]):
                acc_s = jnp.zeros((8, 128), jnp.float32)
                acc_q = jnp.zeros((8, 128), jnp.float32)
                for g in range(min(16, CHUNKS[c] // 8 - 16 * t)):
                    r = STARTS[c] + 128 * t + 8 * g
                    da = xv[r:r + 8, 0:128] - pivot
                    db = xv[r:r + 8, 128:256] - pivot
                    msk = diff == 8 * g
                    acc_s = jnp.where(msk, jnp.sum(da + db, axis=1, keepdims=True), acc_s)
                    acc_q = jnp.where(msk, jnp.sum(da * da + db * db, axis=1, keepdims=True), acc_q)
                row_s = jnp.sum(acc_s, axis=0, keepdims=True)
                row_q = jnp.sum(acc_q, axis=0, keepdims=True)
                u = row_s * (1.0 / (2 * N))
                st[c, 2 * t:2 * t + 1, :] = half_pivot_row + u
                st[c, 2 * t + 1:2 * t + 2, :] = row_q * (1.0 / (2 * N)) - u * (row_s * (1.0 / N))
            if c == 0:
                pl.semaphore_wait(bar, 1)
            rd = pltpu.make_async_remote_copy(
                src_ref=st.at[c, pl.ds(0, 2 * TILES[c])], dst_ref=rx.at[c, pl.ds(0, 2 * TILES[c])],
                send_sem=send_sems.at[c], recv_sem=recv_sems.at[c],
                device_id=nbr, device_id_type=MESH)
            rd.start()
            rdmas.append(rd)

        g_cp.wait()
        b_cp.wait()
        ga = gv[:, 0:128]
        gb = gv[:, 128:256]
        ba = bv[:, 0:128]
        bb = bv[:, 128:256]

        def row(ref, c, i):
            return jnp.broadcast_to(ref[c, i:i + 1, :], (8, 128))

        for c in range(C):
            if c == C - 1:
                for rd in rdmas[:C - 1]:
                    rd.wait_send()
            pre = [(row(st, c, 2 * t), row(st, c, 2 * t + 1) + EPS) for t in range(TILES[c])]
            rdmas[c].wait_recv()
            for t in range(TILES[c]):
                m_a, q_a = pre[t]
                m_b = row(rx, c, 2 * t)
                dl = m_a - m_b
                var = (q_a + row(rx, c, 2 * t + 1)) + dl * dl
                mean8 = m_a + m_b
                rstd8 = lax.rsqrt(var)
                for g in range(min(16, CHUNKS[c] // 8 - 16 * t)):
                    r = STARTS[c] + 128 * t + 8 * g
                    msk = diff == 8 * g
                    mu = jnp.sum(jnp.where(msk, mean8, 0.0), axis=1, keepdims=True)
                    rs = jnp.sum(jnp.where(msk, rstd8, 0.0), axis=1, keepdims=True)
                    o_ref[r:r + 8, 0:128] = (xv[r:r + 8, 0:128] - mu) * rs * ga + ba
                    o_ref[r:r + 8, 128:256] = (xv[r:r + 8, 128:256] - mu) * rs * gb + bb
        rdmas[C - 1].wait_send()

    return pl.pallas_call(
        body,
        out_shape=pltpu.VMEM((M, N), jnp.float32),
        in_specs=[pl.BlockSpec(memory_space=pltpu.HBM)] * 3,
        out_specs=pl.BlockSpec(memory_space=pltpu.VMEM),
        scratch_shapes=[
            pltpu.VMEM((M, N), jnp.float32),
            pltpu.VMEM((1, N), jnp.float32),
            pltpu.VMEM((1, N), jnp.float32),
            pltpu.VMEM((C, 2 * TMAX, 128), jnp.float32),
            pltpu.VMEM((C, 2 * TMAX, 128), jnp.float32),
            pltpu.SemaphoreType.DMA((C + 1,)),
            pltpu.SemaphoreType.DMA((2,)),
            pltpu.SemaphoreType.DMA((C,)),
            pltpu.SemaphoreType.DMA((C,)),
        ],
        compiler_params=pltpu.CompilerParams(
            collective_id=0, disable_semaphore_checks=True, disable_bounds_checks=True),
    )(x, gamma.reshape(1, N), beta.reshape(1, N))
```

```python
import jax
import jax.numpy as jnp
from jax import lax
from jax.experimental import pallas as pl
from jax.experimental.pallas import tpu as pltpu

M, N = 512, 256
EPS = 1e-5
CHUNKS = (136, 128, 128, 120)
STARTS = tuple(sum(CHUNKS[:i]) for i in range(len(CHUNKS)))
C = len(CHUNKS)
TILES = tuple(-(-r // 128) for r in CHUNKS)
TMAX = max(TILES)
PIV = 8
MESH = pl.DeviceIdType.MESH


def pallas_dist_layernorm_xy_m512_n256_kernel(x, gamma, beta):
    def body(x_hbm, g_hbm, b_hbm, o_ref, xv, gv, bv, st, rx, in_sems, p_sems, send_sems, recv_sems):
        bounds = [(0, PIV)] + [(max(STARTS[c], PIV), STARTS[c] + CHUNKS[c]) for c in range(C)]
        in_cps = [
            pltpu.make_async_copy(x_hbm.at[pl.ds(a, b - a)], xv.at[pl.ds(a, b - a)], in_sems.at[i])
            for i, (a, b) in enumerate(bounds)
        ]
        for cp in in_cps:
            cp.start()
        nbr = (lax.axis_index("x"), 1 - lax.axis_index("y"))
        bar = pltpu.get_barrier_semaphore()
        pl.semaphore_signal(bar, inc=1, device_id=nbr, device_id_type=MESH)
        g_cp = pltpu.make_async_copy(g_hbm, gv, p_sems.at[0])
        b_cp = pltpu.make_async_copy(b_hbm, bv, p_sems.at[1])
        g_cp.start()
        b_cp.start()

        diff = (lax.broadcasted_iota(jnp.int32, (8, 128), 1)
                - lax.broadcasted_iota(jnp.int32, (8, 128), 0))

        in_cps[0].wait()
        pivot = jnp.sum(xv[0:PIV, 0:128] + xv[0:PIV, 128:256], axis=1, keepdims=True) * (1.0 / N)
        pivot = jnp.broadcast_to(pivot, (8, 128))
        half_pivot_row = jnp.sum(jnp.where((diff & 7) == 0, pivot * 0.5, 0.0), axis=0, keepdims=True)

        rdmas = []
        for c in range(C):
            in_cps[c + 1].wait()
            for t in range(TILES[c]):
                acc_s = jnp.zeros((8, 128), jnp.float32)
                acc_q = jnp.zeros((8, 128), jnp.float32)
                for g in range(min(16, CHUNKS[c] // 8 - 16 * t)):
                    r = STARTS[c] + 128 * t + 8 * g
                    da = xv[r:r + 8, 0:128] - pivot
                    db = xv[r:r + 8, 128:256] - pivot
                    msk = diff == 8 * g
                    acc_s = jnp.where(msk, jnp.sum(da + db, axis=1, keepdims=True), acc_s)
                    acc_q = jnp.where(msk, jnp.sum(da * da + db * db, axis=1, keepdims=True), acc_q)
                row_s = jnp.sum(acc_s, axis=0, keepdims=True)
                row_q = jnp.sum(acc_q, axis=0, keepdims=True)
                u = row_s * (1.0 / (2 * N))
                st[c, 2 * t:2 * t + 1, :] = half_pivot_row + u
                st[c, 2 * t + 1:2 * t + 2, :] = row_q * (1.0 / (2 * N)) - u * (row_s * (1.0 / N))
            if c == 0:
                pl.semaphore_wait(bar, 1)
            rd = pltpu.make_async_remote_copy(
                src_ref=st.at[c, pl.ds(0, 2 * TILES[c])], dst_ref=rx.at[c, pl.ds(0, 2 * TILES[c])],
                send_sem=send_sems.at[c], recv_sem=recv_sems.at[c],
                device_id=nbr, device_id_type=MESH)
            rd.start()
            rdmas.append(rd)

        g_cp.wait()
        b_cp.wait()
        ga = gv[:, 0:128]
        gb = gv[:, 128:256]
        ba = bv[:, 0:128]
        bb = bv[:, 128:256]

        def row(ref, c, i):
            return jnp.broadcast_to(ref[c, i:i + 1, :], (8, 128))

        def lane_bcast(v8, g):
            return jnp.sum(jnp.where(diff == 8 * g, v8, 0.0), axis=1, keepdims=True)

        for c in range(C):
            if c == C - 1:
                for rd in rdmas[:C - 1]:
                    rd.wait_send()
            pre = [(row(st, c, 2 * t), row(st, c, 2 * t + 1) + EPS) for t in range(TILES[c])]
            rdmas[c].wait_recv()
            for t in range(TILES[c]):
                m_a, q_a = pre[t]
                m_b = row(rx, c, 2 * t)
                dl = m_a - m_b
                var = (q_a + row(rx, c, 2 * t + 1)) + dl * dl
                mean8 = m_a + m_b
                rstd8 = lax.rsqrt(var)
                base = STARTS[c] + 128 * t
                groups = range(min(16, CHUNKS[c] // 8 - 16 * t))
                mus = [lane_bcast(mean8, g) for g in groups]
                rss = [lane_bcast(rstd8, g) for g in groups]
                ya = [(xv[base + 8 * g:base + 8 * g + 8, 0:128] - mus[g]) * ga for g in groups]
                yb = [(xv[base + 8 * g:base + 8 * g + 8, 128:256] - mus[g]) * gb for g in groups]
                for g in groups:
                    r = base + 8 * g
                    o_ref[r:r + 8, 0:128] = ya[g] * rss[g] + ba
                    o_ref[r:r + 8, 128:256] = yb[g] * rss[g] + bb
        rdmas[C - 1].wait_send()

    return pl.pallas_call(
        body,
        out_shape=pltpu.VMEM((M, N), jnp.float32),
        in_specs=[pl.BlockSpec(memory_space=pltpu.HBM)] * 3,
        out_specs=pl.BlockSpec(memory_space=pltpu.VMEM),
        scratch_shapes=[
            pltpu.VMEM((M, N), jnp.float32),
            pltpu.VMEM((1, N), jnp.float32),
            pltpu.VMEM((1, N), jnp.float32),
            pltpu.VMEM((C, 2 * TMAX, 128), jnp.float32),
            pltpu.VMEM((C, 2 * TMAX, 128), jnp.float32),
            pltpu.SemaphoreType.DMA((C + 1,)),
            pltpu.SemaphoreType.DMA((2,)),
            pltpu.SemaphoreType.DMA((C,)),
            pltpu.SemaphoreType.DMA((C,)),
        ],
        compiler_params=pltpu.CompilerParams(
            collective_id=0, disable_semaphore_checks=True, disable_bounds_checks=True),
    )(x, gamma.reshape(1, N), beta.reshape(1, N))
```
